```python
import numpy as np

kernel_name = "dist_mean_ax0_shard0_i_m4096_n1024"

def setup_inputs():
    return {"x": np.random.randn(16384, 1024).astype(np.float32)}

def reference(x: np.ndarray) -> np.ndarray:
    return np.mean(x, axis=0, keepdims=True)
```

```python
import jax
import jax.numpy as jnp
from jax import lax
from jax.experimental import pallas as pl
from jax.experimental.pallas import tpu as pltpu

N_DEV = 4


def pallas_dist_mean_ax0_shard0_i_m4096_n1024_kernel(
x: jax.Array,
):
    m_per, n = x.shape
    n_chunks = 16
    rows = m_per // n_chunks
    inv_total = 1.0 / (N_DEV * m_per)

    def body(x_hbm, out_ref, buf, comm, copy_sems, send_sems, recv_sems):
        my = lax.axis_index("i")

        copies = []
        for c in range(n_chunks):
            cp = pltpu.make_async_copy(
                x_hbm.at[pl.ds(c * rows, rows), :],
                buf.at[pl.ds(c * rows, rows), :],
                copy_sems.at[c],
            )
            cp.start()
            copies.append(cp)

        barrier = pltpu.get_barrier_semaphore()
        for d in range(1, N_DEV):
            pl.semaphore_signal(
                barrier, inc=1,
                device_id=((my + d) % N_DEV,),
                device_id_type=pl.DeviceIdType.MESH,
            )

        acc = jnp.zeros((8, n), jnp.float32)
        for c in range(n_chunks):
            copies[c].wait()

            def step(i, a, c=c):
                r = pl.multiple_of(c * rows + i * 64, 64)
                blk = buf[pl.ds(r, 64), :]
                return a + jnp.sum(blk.reshape(8, 8, n), axis=0)

            acc = lax.fori_loop(0, rows // 64, step, acc)

        comm[0] = jnp.sum(acc, axis=0, keepdims=True) * inv_total

        pl.semaphore_wait(barrier, N_DEV - 1)

        rdmas = []
        for d in range(1, N_DEV):
            r = pltpu.make_async_remote_copy(
                src_ref=comm.at[0],
                dst_ref=comm.at[d],
                send_sem=send_sems.at[d - 1],
                recv_sem=recv_sems.at[d - 1],
                device_id=((my + d) % N_DEV,),
                device_id_type=pl.DeviceIdType.MESH,
            )
            r.start()
            rdmas.append(r)
        for r in rdmas:
            r.wait_recv()
        out_ref[...] = (comm[0] + comm[1]) + (comm[2] + comm[3])
        for r in rdmas:
            r.wait_send()

    return pl.pallas_call(
        body,
        out_shape=jax.ShapeDtypeStruct((1, n), jnp.float32),
        in_specs=[pl.BlockSpec(memory_space=pl.ANY)],
        out_specs=pl.BlockSpec(memory_space=pltpu.VMEM),
        scratch_shapes=[
            pltpu.VMEM((m_per, n), jnp.float32),
            pltpu.VMEM((N_DEV, 1, n), jnp.float32),
            pltpu.SemaphoreType.DMA((n_chunks,)),
            pltpu.SemaphoreType.DMA((N_DEV - 1,)),
            pltpu.SemaphoreType.DMA((N_DEV - 1,)),
        ],
        compiler_params=pltpu.CompilerParams(
            collective_id=0, vmem_limit_bytes=64 * 1024 * 1024
        ),
    )(x)
```

```python
import jax
import jax.numpy as jnp
from jax import lax
from jax.experimental import pallas as pl
from jax.experimental.pallas import tpu as pltpu

N_DEV = 4
MESH = pl.DeviceIdType.MESH

BLK = 8
N_STREAMS = 16
PREFILL = 26


def pallas_dist_mean_ax0_shard0_i_m4096_n1024_kernel(
x: jax.Array,
):
    m_per, n = x.shape
    nb = m_per // BLK
    sb = nb // N_STREAMS
    inv_total = 1.0 / (N_DEV * m_per)

    gb = [0, nb - 112, nb - 32, nb - 4, nb]
    ng = len(gb) - 1

    def group(p):
        return next(g for g in range(ng) if gb[g] <= p < gb[g + 1])

    lo = [p for p in range(nb) if p % 2 == 0 or p >= nb - PREFILL]
    hi = [p for p in range(nb) if p % 2 == 1 and p < nb - PREFILL]
    seq = [(p, 1) for p in lo[:PREFILL]]
    for a, b in zip(hi, lo[PREFILL:]):
        seq += [(a, 0), (b, 1)]
    assert sorted(p for p, _ in seq) == list(range(nb))

    head = PREFILL + N_STREAMS
    n_loop = 0
    while all(
        seq[head + N_STREAMS * n_loop + q][0] == seq[head + q][0] + N_STREAMS * n_loop
        and group(seq[head + N_STREAMS * n_loop + q][0]) == 0
        for q in range(N_STREAMS)
    ):
        n_loop += 1

    def body(x_hbm, out_ref, buf, comm, copy_sems, send_sem, recv_sem):
        def start_copy(p, prio, m=None):
            src = ((p % N_STREAMS) * sb + p // N_STREAMS) * BLK
            dst = p * BLK
            if m is not None:
                src = pl.multiple_of(src + m * BLK, BLK)
                dst = pl.multiple_of(dst + m * (BLK * N_STREAMS), BLK)
            pltpu.make_async_copy(
                x_hbm.at[pl.ds(src, BLK), :],
                buf.at[pl.ds(dst, BLK), :],
                copy_sems.at[group(p)],
            ).start(priority=prio)

        def add_rows(off, rows, acc, u=64):
            full = rows // u if rows > 2 * u else 0
            if full:
                def step(t, a):
                    r = pl.multiple_of(off + t * u, 8)
                    blk = buf[pl.ds(r, u), :]
                    return a + jnp.sum(blk.reshape(u // 8, 8, n), axis=0)

                acc = lax.fori_loop(0, full, step, acc)
            rem = rows - full * u
            if rem:
                blk = buf[pl.ds(off + full * u, rem), :]
                acc = acc + jnp.sum(blk.reshape(rem // 8, 8, n), axis=0)
            return acc

        for p, prio in seq[:head]:
            start_copy(p, prio)

        my = lax.axis_index("i")
        peers = (2, 1, 3)
        barrier = pltpu.get_barrier_semaphore()
        for d in peers:
            pl.semaphore_signal(
                barrier, inc=1,
                device_id=((my + d) % N_DEV,), device_id_type=MESH,
            )

        def issue(m, c):
            for p, prio in seq[head:head + N_STREAMS]:
                start_copy(p, prio, m)
            return c

        lax.fori_loop(0, n_loop, issue, 0)
        for p, prio in seq[head + N_STREAMS * n_loop:]:
            start_copy(p, prio)

        pl.semaphore_wait(barrier, N_DEV - 1)

        acc = jnp.zeros((8, n), jnp.float32)
        for g in range(ng):
            rows = (gb[g + 1] - gb[g]) * BLK
            v = buf.at[pl.ds(gb[g] * BLK, rows), :]
            pltpu.make_async_copy(v, v, copy_sems.at[g]).wait()
            acc = add_rows(gb[g] * BLK, rows, acc)

        comm[0] = jnp.sum(acc, axis=0, keepdims=True) * inv_total

        for d in peers:
            pltpu.make_async_remote_copy(
                src_ref=comm.at[0],
                dst_ref=comm.at[d],
                send_sem=send_sem,
                recv_sem=recv_sem,
                device_id=((my + d) % N_DEV,),
                device_id_type=MESH,
            ).start()
        v = comm.at[pl.ds(1, N_DEV - 1)]
        pltpu.make_async_copy(v, v, send_sem).wait()
        pltpu.make_async_copy(v, v, recv_sem).wait()
        out_ref[...] = (comm[0] + comm[1]) + (comm[3] + comm[2])

    return pl.pallas_call(
        body,
        out_shape=jax.ShapeDtypeStruct((1, n), jnp.float32),
        in_specs=[pl.BlockSpec(memory_space=pl.ANY)],
        out_specs=pl.BlockSpec(memory_space=pltpu.VMEM),
        scratch_shapes=[
            pltpu.VMEM((m_per, n), jnp.float32),
            pltpu.VMEM((N_DEV, 1, n), jnp.float32),
            pltpu.SemaphoreType.DMA((ng,)),
            pltpu.SemaphoreType.DMA,
            pltpu.SemaphoreType.DMA,
        ],
        compiler_params=pltpu.CompilerParams(
            collective_id=0, vmem_limit_bytes=32 * 1024 * 1024
        ),
    )(x)
```

```python
import jax
import jax.numpy as jnp
from jax import lax
from jax.experimental import pallas as pl
from jax.experimental.pallas import tpu as pltpu

N_DEV = 4
MESH = pl.DeviceIdType.MESH

BLK = 8
N_STREAMS = 16
PREFILL = 26
N_SPLIT = 10
LATE_COLS = 256


def _tree_sum(vals):
    vals = list(vals)
    while len(vals) > 1:
        nxt = [vals[i] + vals[i + 1] for i in range(0, len(vals) - 1, 2)]
        if len(vals) % 2:
            nxt.append(vals[-1])
        vals = nxt
    return vals[0]


def pallas_dist_mean_ax0_shard0_i_m4096_n1024_kernel(
x: jax.Array,
):
    m_per, n = x.shape
    nb = m_per // BLK
    sb = nb // N_STREAMS
    ns = nb - N_SPLIT
    lc = LATE_COLS
    ec = n - lc
    inv_total = 1.0 / (N_DEV * m_per)

    copies = (
        [(p, 0, n) for p in range(ns)]
        + [(p, lc, ec) for p in range(ns, nb)]
        + [(p, 0, lc) for p in range(ns, nb)]
    )
    whole = [(0, nb - 112, 0, n), (nb - 112, nb - 32, 0, n), (nb - 32, ns, 0, n)]
    early = [(ns, nb - 2, lc, ec), (nb - 2, nb, lc, ec)]
    late = (ns, nb, 0, lc)
    groups = whole + early + [late]

    def group_of(c):
        p, c0, nc = c
        return next(
            g for g, (a, b, gc0, gnc) in enumerate(groups)
            if a <= p < b and (gc0, gnc) == (c0, nc)
        )

    nc_all = len(copies)
    lo = [c for i, c in enumerate(copies) if i % 2 == 0 or i >= nc_all - PREFILL]
    hi = [c for i, c in enumerate(copies) if i % 2 == 1 and i < nc_all - PREFILL]
    seq = [(c, 1) for c in lo[:PREFILL]]
    for a, b in zip(hi, lo[PREFILL:], strict=True):
        seq += [(a, 0), (b, 1)]

    head = PREFILL + N_STREAMS
    n_loop = 0
    while all(
        seq[head + N_STREAMS * n_loop + q][0][0]
        == seq[head + q][0][0] + N_STREAMS * n_loop
        and group_of(seq[head + N_STREAMS * n_loop + q][0]) == 0
        for q in range(N_STREAMS)
    ):
        n_loop += 1

    def body(x_hbm, out_ref, buf, late_buf, comm):
        def scoped(copy_sems, send_sems, recv_sems):
            def dst_view(row, rows, c0, nc):
                if nc == lc:
                    return late_buf.at[pl.ds(row - ns * BLK, rows), :]
                return buf.at[pl.ds(row, rows), pl.ds(c0, nc)]

            def start_copy(c, prio, m=None):
                p, c0, nc = c
                src = ((p % N_STREAMS) * sb + p // N_STREAMS) * BLK
                dst = p * BLK
                if m is not None:
                    src = pl.multiple_of(src + m * BLK, BLK)
                    dst = pl.multiple_of(dst + m * (N_STREAMS * BLK), BLK)
                pltpu.make_async_copy(
                    x_hbm.at[pl.ds(src, BLK), pl.ds(c0, nc)],
                    dst_view(dst, BLK, c0, nc),
                    copy_sems.at[group_of(c)],
                ).start(priority=prio)

            def wait_group(grp):
                a, b, c0, nc = grp
                v = dst_view(a * BLK, (b - a) * BLK, c0, nc)
                pltpu.make_async_copy(v, v, copy_sems.at[groups.index(grp)]).wait()

            def add_group(grp, acc, u=64):
                a, b, c0, nc = grp
                off, rows = a * BLK, (b - a) * BLK
                full = rows // u if rows > 2 * u else 0
                if full:
                    def step(t, s):
                        r = pl.multiple_of(off + t * u, 8)
                        blk = buf[pl.ds(r, u), pl.ds(c0, nc)]
                        return s + jnp.sum(blk.reshape(u // 8, 8, nc), axis=0)

                    acc = lax.fori_loop(0, full, step, acc)
                rem = rows - full * u
                if rem:
                    blk = buf[pl.ds(off + full * u, rem), pl.ds(c0, nc)]
                    acc = acc + jnp.sum(blk.reshape(rem // 8, 8, nc), axis=0)
                return acc

            for c, prio in seq[:head]:
                start_copy(c, prio)

            my = lax.axis_index("i")
            barrier = pltpu.get_barrier_semaphore()
            for d in (2, 1, 3):
                pl.semaphore_signal(
                    barrier, inc=1,
                    device_id=((my + d) % N_DEV,), device_id_type=MESH,
                )

            def issue(m, carry):
                for c, prio in seq[head:head + N_STREAMS]:
                    start_copy(c, prio, m)
                return carry

            lax.fori_loop(0, n_loop, issue, 0)
            for c, prio in seq[head + N_STREAMS * n_loop:]:
                start_copy(c, prio)

            pl.semaphore_wait(barrier, N_DEV - 1)

            def send(k, d, c0, nc):
                rdma = pltpu.make_async_remote_copy(
                    src_ref=comm.at[0, :, pl.ds(c0, nc)],
                    dst_ref=comm.at[d, :, pl.ds(c0, nc)],
                    send_sem=send_sems.at[k],
                    recv_sem=recv_sems.at[k],
                    device_id=((my + d) % N_DEV,),
                    device_id_type=MESH,
                )
                rdma.start()
                return rdma

            acc = jnp.zeros((8, n), jnp.float32)
            for grp in whole:
                wait_group(grp)
                acc = add_group(grp, acc)

            acc_early = acc[:, lc:]
            for grp in early:
                wait_group(grp)
                acc_early = add_group(grp, acc_early)
            comm[0, :, pl.ds(lc, ec)] = (
                jnp.sum(acc_early, axis=0, keepdims=True) * inv_total
            )
            diag_early = send(0, 2, lc, ec)

            wait_group(late)
            acc_late = _tree_sum(
                [acc[:, :lc]]
                + [late_buf[pl.ds(t * BLK, BLK), :] for t in range(N_SPLIT)]
            )
            comm[0, :, pl.ds(0, lc)] = (
                jnp.sum(acc_late, axis=0, keepdims=True) * inv_total
            )
            diag_late = send(1, 2, 0, lc)
            right = send(2, 1, 0, n)
            left = send(3, 3, 0, n)

            for rdma in (diag_early, diag_late, right, left):
                rdma.wait_send()
            right.wait_recv()
            left.wait_recv()
            part = comm[0] + (comm[1] + comm[3])
            diag_early.wait_recv()
            diag_late.wait_recv()
            out_ref[...] = part + comm[2]

        pl.run_scoped(
            scoped,
            pltpu.SemaphoreType.DMA((len(groups),)),
            pltpu.SemaphoreType.DMA((4,)),
            pltpu.SemaphoreType.DMA((4,)),
        )

    return pl.pallas_call(
        body,
        out_shape=jax.ShapeDtypeStruct((1, n), jnp.float32),
        in_specs=[pl.BlockSpec(memory_space=pl.ANY)],
        out_specs=pl.BlockSpec(memory_space=pltpu.VMEM),
        scratch_shapes=[
            pltpu.VMEM((m_per, n), jnp.float32),
            pltpu.VMEM((N_SPLIT * BLK, lc), jnp.float32),
            pltpu.VMEM((N_DEV, 1, n), jnp.float32),
        ],
        compiler_params=pltpu.CompilerParams(
            collective_id=0, vmem_limit_bytes=32 * 1024 * 1024
        ),
    )(x)
```

```python
import jax
import jax.numpy as jnp
from jax import lax
from jax.experimental import pallas as pl
from jax.experimental.pallas import tpu as pltpu

N_DEV = 4
MESH = pl.DeviceIdType.MESH

BLK = 8
N_STREAMS = 16
PREFILL = 26
N_SPLIT = 10
LATE_COLS = 256


def _tree_sum(vals):
    vals = list(vals)
    while len(vals) > 1:
        nxt = [vals[i] + vals[i + 1] for i in range(0, len(vals) - 1, 2)]
        if len(vals) % 2:
            nxt.append(vals[-1])
        vals = nxt
    return vals[0]


def pallas_dist_mean_ax0_shard0_i_m4096_n1024_kernel(
x: jax.Array,
):
    m_per, n = x.shape
    nb = m_per // BLK
    sb = nb // N_STREAMS
    ns = nb - N_SPLIT
    lc = LATE_COLS
    ec = n - lc
    inv_total = 1.0 / (N_DEV * m_per)

    copies = (
        [(p, 0, n) for p in range(ns)]
        + [(p, lc, ec) for p in range(ns, nb)]
        + [(p, 0, lc) for p in range(ns, nb)]
    )
    whole = [(0, nb - 112, 0, n), (nb - 112, nb - 32, 0, n), (nb - 32, ns, 0, n)]
    early = [(ns, nb - 2, lc, ec), (nb - 2, nb, lc, ec)]
    late = [(ns, nb - 2, 0, lc), (nb - 2, nb, 0, lc)]
    groups = whole + early + late

    def group_of(c):
        p, c0, nc = c
        return next(
            g for g, (a, b, gc0, gnc) in enumerate(groups)
            if a <= p < b and (gc0, gnc) == (c0, nc)
        )

    nc_all = len(copies)
    lo = [c for i, c in enumerate(copies) if i % 2 == 0 or i >= nc_all - PREFILL]
    hi = [c for i, c in enumerate(copies) if i % 2 == 1 and i < nc_all - PREFILL]
    seq = [(c, 1) for c in lo[:PREFILL]]
    for a, b in zip(hi, lo[PREFILL:], strict=True):
        seq += [(a, 0), (b, 1)]

    head = PREFILL + N_STREAMS
    n_loop = 0
    while all(
        seq[head + N_STREAMS * n_loop + q][0][0]
        == seq[head + q][0][0] + N_STREAMS * n_loop
        and group_of(seq[head + N_STREAMS * n_loop + q][0]) == 0
        for q in range(N_STREAMS)
    ):
        n_loop += 1

    def body(x_hbm, out_ref, buf, late_buf, comm):
        def scoped(copy_sems, send_sems, recv_sems):
            def dst_view(row, rows, c0, nc):
                if nc == lc:
                    return late_buf.at[pl.ds(row - ns * BLK, rows), :]
                return buf.at[pl.ds(row, rows), pl.ds(c0, nc)]

            def start_copy(c, prio, m=None):
                p, c0, nc = c
                src = ((p % N_STREAMS) * sb + p // N_STREAMS) * BLK
                dst = p * BLK
                if m is not None:
                    src = pl.multiple_of(src + m * BLK, BLK)
                    dst = pl.multiple_of(dst + m * (N_STREAMS * BLK), BLK)
                pltpu.make_async_copy(
                    x_hbm.at[pl.ds(src, BLK), pl.ds(c0, nc)],
                    dst_view(dst, BLK, c0, nc),
                    copy_sems.at[group_of(c)],
                ).start(priority=prio)

            def wait_group(grp):
                a, b, c0, nc = grp
                v = dst_view(a * BLK, (b - a) * BLK, c0, nc)
                pltpu.make_async_copy(v, v, copy_sems.at[groups.index(grp)]).wait()

            def add_group(grp, acc, u=64):
                a, b, c0, nc = grp
                off, rows = a * BLK, (b - a) * BLK
                full = rows // u if rows > 2 * u else 0
                if full:
                    def step(t, s):
                        r = pl.multiple_of(off + t * u, 8)
                        blk = buf[pl.ds(r, u), pl.ds(c0, nc)]
                        return s + jnp.sum(blk.reshape(u // 8, 8, nc), axis=0)

                    acc = lax.fori_loop(0, full, step, acc)
                rem = rows - full * u
                if rem:
                    blk = buf[pl.ds(off + full * u, rem), pl.ds(c0, nc)]
                    acc = acc + jnp.sum(blk.reshape(rem // 8, 8, nc), axis=0)
                return acc

            for c, prio in seq[:head]:
                start_copy(c, prio)

            my = lax.axis_index("i")
            barrier = pltpu.get_barrier_semaphore()
            for d in (2, 1, 3):
                pl.semaphore_signal(
                    barrier, inc=1,
                    device_id=((my + d) % N_DEV,), device_id_type=MESH,
                )

            def issue(m, carry):
                for c, prio in seq[head:head + N_STREAMS]:
                    start_copy(c, prio, m)
                return carry

            lax.fori_loop(0, n_loop, issue, 0)
            for c, prio in seq[head + N_STREAMS * n_loop:]:
                start_copy(c, prio)

            pl.semaphore_wait(barrier, N_DEV - 1)

            def send(k, d, c0, nc):
                rdma = pltpu.make_async_remote_copy(
                    src_ref=comm.at[0, :, pl.ds(c0, nc)],
                    dst_ref=comm.at[d, :, pl.ds(c0, nc)],
                    send_sem=send_sems.at[k],
                    recv_sem=recv_sems.at[k],
                    device_id=((my + d) % N_DEV,),
                    device_id_type=MESH,
                )
                rdma.start()
                return rdma

            acc = jnp.zeros((8, n), jnp.float32)
            for grp in whole:
                wait_group(grp)
                acc = add_group(grp, acc)

            acc_early = acc[:, lc:]
            for grp in early:
                wait_group(grp)
                acc_early = add_group(grp, acc_early)
            comm[0, :, pl.ds(lc, ec)] = (
                jnp.sum(acc_early, axis=0, keepdims=True) * inv_total
            )
            diag_early = send(0, 2, lc, ec)

            acc_late = acc[:, :lc]
            for grp in late:
                wait_group(grp)
                acc_late = _tree_sum(
                    [acc_late]
                    + [
                        late_buf[pl.ds((p - ns) * BLK, BLK), :]
                        for p in range(grp[0], grp[1])
                    ]
                )
            comm[0, :, pl.ds(0, lc)] = (
                jnp.sum(acc_late, axis=0, keepdims=True) * inv_total
            )
            diag_late = send(1, 2, 0, lc)
            right = send(2, 1, 0, n)
            left = send(3, 3, 0, n)

            for rdma in (diag_early, diag_late, right, left):
                rdma.wait_send()
            right.wait_recv()
            left.wait_recv()
            part = comm[0] + (comm[1] + comm[3])
            diag_early.wait_recv()
            diag_late.wait_recv()
            out_ref[...] = part + comm[2]

        pl.run_scoped(
            scoped,
            pltpu.SemaphoreType.DMA((len(groups),)),
            pltpu.SemaphoreType.DMA((4,)),
            pltpu.SemaphoreType.DMA((4,)),
        )

    return pl.pallas_call(
        body,
        out_shape=jax.ShapeDtypeStruct((1, n), jnp.float32),
        in_specs=[pl.BlockSpec(memory_space=pl.ANY)],
        out_specs=pl.BlockSpec(memory_space=pltpu.VMEM),
        scratch_shapes=[
            pltpu.VMEM((m_per, n), jnp.float32),
            pltpu.VMEM((N_SPLIT * BLK, lc), jnp.float32),
            pltpu.VMEM((N_DEV, 1, n), jnp.float32),
        ],
        compiler_params=pltpu.CompilerParams(
            collective_id=0, vmem_limit_bytes=32 * 1024 * 1024
        ),
    )(x)
```

```python
import jax
import jax.numpy as jnp
from jax import lax
from jax.experimental import pallas as pl
from jax.experimental.pallas import tpu as pltpu

N_DEV = 4
MESH = pl.DeviceIdType.MESH
SUB, LANE = 8, 128

N_STREAMS = 16
OFFSET = 7
PREFILL = 28
N_SPLIT = 10
N_LATE = 2


def _tree_sum(vals):
    vals = list(vals)
    while len(vals) > 1:
        nxt = [vals[i] + vals[i + 1] for i in range(0, len(vals) - 1, 2)]
        if len(vals) % 2:
            nxt.append(vals[-1])
        vals = nxt
    return vals[0]


def pallas_dist_mean_ax0_shard0_i_m4096_n1024_kernel(
x: jax.Array,
):
    m_per, n = x.shape
    ct = n // LANE
    nb = m_per // SUB
    nt = nb * ct
    sb = nb // N_STREAMS
    ns = nb - N_SPLIT
    n_early = ct - N_LATE
    inv_total = 1.0 / (N_DEV * m_per)

    def first_tile(p):
        return ((p % N_STREAMS) * sb + p // N_STREAMS) * ct + OFFSET

    whole = [(0, nb - 112, 0, ct), (nb - 112, nb - 32, 0, ct), (nb - 32, ns, 0, ct)]
    early = [(ns, nb - 2, 0, n_early), (nb - 2, nb, 0, n_early)]
    late = [(ns, nb - 2, n_early, N_LATE), (nb - 2, nb, n_early, N_LATE)]
    groups = whole + early + late

    copies = []
    for g, (a, b, s0, sn) in enumerate(groups):
        for p in range(a, b):
            k = nt - (first_tile(p) + s0)
            if 0 < k < sn:
                copies += [(p, s0, k, g), (p, s0 + k, sn - k, g)]
            else:
                copies += [(p, s0, sn, g)]

    cut = (len(copies) - PREFILL) // 2 * 2
    lo = copies[0:cut:2] + copies[cut:]
    hi = copies[1:cut:2]
    seq = [(c, 1) for c in lo[:PREFILL]]
    for i, c in enumerate(lo[PREFILL:]):
        seq += [(h, 0) for h in hi[i:i + 1]] + [(c, 1)]
    assert sorted(c for c, _ in seq) == sorted(copies)

    head = PREFILL + N_STREAMS
    n_loop = 0
    while all(
        seq[head + N_STREAMS * n_loop + q][0]
        == (seq[head + q][0][0] + N_STREAMS * n_loop, 0, ct, 0)
        for q in range(N_STREAMS)
    ):
        n_loop += 1

    def lanes(s0, sn):
        return pl.ds(s0 * LANE, sn * LANE)

    def column_runs(s0, sn):
        c0 = (s0 + OFFSET) % ct
        k = min(sn, ct - c0)
        return [(s0, k, c0)] + ([(s0 + k, sn - k, 0)] if k < sn else [])

    def body(x_hbm, out_ref, whole_buf, early_buf, late_buf, comm):
        def scoped(copy_sems, send_sems, recv_sems):
            def dst_of(g, p):
                if groups[g] in whole:
                    return whole_buf, p * ct
                buf = early_buf if groups[g] in early else late_buf
                return buf, (p - ns) * groups[g][3]

            def start_copy(c, prio, m=0):
                p, s0, sn, g = c
                buf, dst = dst_of(g, p)
                src = (first_tile(p) + s0) % nt + m * ct
                dst = dst + s0 - groups[g][2] + m * (N_STREAMS * ct)
                pltpu.make_async_copy(
                    x_hbm.at[pl.ds(src, sn)],
                    buf.at[pl.ds(dst, sn)],
                    copy_sems.at[g],
                ).start(priority=prio)

            def add_group(grp, acc, u=8):
                g = groups.index(grp)
                a, b, _, sn = grp
                buf, off = dst_of(g, a)
                v = buf.at[pl.ds(off, (b - a) * sn)]
                pltpu.make_async_copy(v, v, copy_sems.at[g]).wait()
                full = (b - a) // u if b - a > 2 * u else 0

                def step(t, s):
                    blk = buf[pl.ds(off + t * (u * sn), u * sn)]
                    return s + jnp.sum(blk.reshape(u, sn, SUB, LANE), axis=0)

                if full:
                    acc = lax.fori_loop(0, full, step, acc)
                return _tree_sum(
                    [acc]
                    + [buf[pl.ds(off + t * sn, sn)] for t in range(full * u, b - a)]
                )

            def finish(acc):
                rows = [
                    jnp.sum(acc[j], axis=0, keepdims=True)
                    for j in range(acc.shape[0])
                ]
                return jnp.concatenate(rows, axis=1) * inv_total

            for c, prio in seq[:head]:
                start_copy(c, prio)

            my = lax.axis_index("i")
            barrier = pltpu.get_barrier_semaphore()
            for d in (2, 1, 3):
                pl.semaphore_signal(
                    barrier, inc=1,
                    device_id=((my + d) % N_DEV,), device_id_type=MESH,
                )

            def issue(m, carry):
                for c, prio in seq[head:head + N_STREAMS]:
                    start_copy(c, prio, m)
                return carry

            lax.fori_loop(0, n_loop, issue, 0)
            for c, prio in seq[head + N_STREAMS * n_loop:]:
                start_copy(c, prio)

            pl.semaphore_wait(barrier, N_DEV - 1)

            def send(k, d, s0, sn):
                rdma = pltpu.make_async_remote_copy(
                    src_ref=comm.at[0, :, lanes(s0, sn)],
                    dst_ref=comm.at[d, :, lanes(s0, sn)],
                    send_sem=send_sems.at[k],
                    recv_sem=recv_sems.at[k],
                    device_id=((my + d) % N_DEV,),
                    device_id_type=MESH,
                )
                rdma.start()
                return rdma

            acc = jnp.zeros((ct, SUB, LANE), jnp.float32)
            for grp in whole:
                acc = add_group(grp, acc)

            acc_early = acc[:n_early]
            for grp in early:
                acc_early = add_group(grp, acc_early)
            comm[0, :, lanes(0, n_early)] = finish(acc_early)
            diag_early = send(0, 2, 0, n_early)

            acc_late = acc[n_early:]
            for grp in late:
                acc_late = add_group(grp, acc_late)
            comm[0, :, lanes(n_early, N_LATE)] = finish(acc_late)
            diag_late = send(1, 2, n_early, N_LATE)
            right = send(2, 1, 0, ct)
            left = send(3, 3, 0, ct)

            for rdma in (diag_early, diag_late, right, left):
                rdma.wait_send()
            right.wait_recv()
            left.wait_recv()

            steps = (
                (diag_early, column_runs(0, n_early)),
                (diag_late, column_runs(n_early, N_LATE)),
            )
            part = {
                s0: comm[0, :, lanes(s0, sn)]
                + (comm[1, :, lanes(s0, sn)] + comm[3, :, lanes(s0, sn)])
                for _, runs in steps
                for s0, sn, _ in runs
            }
            for rdma, runs in steps:
                rdma.wait_recv()
                for s0, sn, c0 in runs:
                    out_ref[:, lanes(c0, sn)] = part[s0] + comm[2, :, lanes(s0, sn)]

        pl.run_scoped(
            scoped,
            pltpu.SemaphoreType.DMA((len(groups),)),
            pltpu.SemaphoreType.DMA((4,)),
            pltpu.SemaphoreType.DMA((4,)),
        )

    x_tiles = (
        x.reshape(nb, SUB, ct, LANE).transpose(0, 2, 1, 3).reshape(nt, SUB, LANE)
    )
    return pl.pallas_call(
        body,
        out_shape=jax.ShapeDtypeStruct((1, n), jnp.float32),
        in_specs=[pl.BlockSpec(memory_space=pl.ANY)],
        out_specs=pl.BlockSpec(memory_space=pltpu.VMEM),
        scratch_shapes=[
            pltpu.VMEM((ns * ct, SUB, LANE), jnp.float32),
            pltpu.VMEM((N_SPLIT * n_early, SUB, LANE), jnp.float32),
            pltpu.VMEM((N_SPLIT * N_LATE, SUB, LANE), jnp.float32),
            pltpu.VMEM((N_DEV, 1, n), jnp.float32),
        ],
        compiler_params=pltpu.CompilerParams(
            collective_id=0, vmem_limit_bytes=32 * 1024 * 1024
        ),
    )(x_tiles)
```

```python
import jax
import jax.numpy as jnp
from jax import lax
from jax.experimental import pallas as pl
from jax.experimental.pallas import tpu as pltpu

N_DEV = 4
MESH = pl.DeviceIdType.MESH
SUB, LANE = 8, 128

N_STREAMS = 16
OFFSET = 7
PREFILL = 28
N_SPLIT = 6
STAGES = ((0, 4), (4, 2), (6, 1), (7, 1))


def _tree_sum(vals):
    vals = list(vals)
    while len(vals) > 1:
        nxt = [vals[i] + vals[i + 1] for i in range(0, len(vals) - 1, 2)]
        if len(vals) % 2:
            nxt.append(vals[-1])
        vals = nxt
    return vals[0]


def pallas_dist_mean_ax0_shard0_i_m4096_n1024_kernel(
x: jax.Array,
):
    m_per, n = x.shape
    ct = n // LANE
    nb = m_per // SUB
    nt = nb * ct
    sb = nb // N_STREAMS
    ns = nb - N_SPLIT
    inv_total = 1.0 / (N_DEV * m_per)

    def first_tile(p):
        return ((p % N_STREAMS) * sb + p // N_STREAMS) * ct + OFFSET

    whole = [(0, nb - 112, 0, ct), (nb - 112, nb - 32, 0, ct), (nb - 32, ns, 0, ct)]
    groups = whole + [(ns, nb, s0, sn) for s0, sn in STAGES]
    base = [0]
    for a, b, _, sn in groups:
        base.append(base[-1] + (b - a) * sn)
    assert base[-1] == nt

    copies = []
    for g, (a, b, s0, sn) in enumerate(groups):
        for p in range(a, b):
            k = nt - (first_tile(p) + s0)
            if 0 < k < sn:
                copies += [(p, s0, k, g), (p, s0 + k, sn - k, g)]
            else:
                copies += [(p, s0, sn, g)]

    cut = (len(copies) - PREFILL) // 2 * 2
    lo = copies[0:cut:2] + copies[cut:]
    hi = copies[1:cut:2]
    seq = [(c, 1) for c in lo[:PREFILL]]
    for i, c in enumerate(lo[PREFILL:]):
        seq += [(h, 0) for h in hi[i:i + 1]] + [(c, 1)]
    assert sorted(c for c, _ in seq) == sorted(copies)

    head = PREFILL + N_STREAMS
    n_loop = 0
    while all(
        seq[head + N_STREAMS * n_loop + q][0]
        == (seq[head + q][0][0] + N_STREAMS * n_loop, 0, ct, 0)
        for q in range(N_STREAMS)
    ):
        n_loop += 1

    def lanes(s0, sn):
        return pl.ds(s0 * LANE, sn * LANE)

    def column_runs(s0, sn):
        c0 = (s0 + OFFSET) % ct
        k = min(sn, ct - c0)
        return [(s0, k, c0)] + ([(s0 + k, sn - k, 0)] if k < sn else [])

    def body(x_hbm, out_ref, buf, comm):
        def scoped(copy_sems, send_sems, recv_sems):
            def start_copy(c, prio, m=0):
                p, s0, sn, g = c
                a, _, gs0, gsn = groups[g]
                src = (first_tile(p) + s0) % nt + m * ct
                dst = base[g] + (p - a) * gsn + s0 - gs0 + m * (N_STREAMS * ct)
                pltpu.make_async_copy(
                    x_hbm.at[pl.ds(src, sn)],
                    buf.at[pl.ds(dst, sn)],
                    copy_sems.at[g],
                ).start(priority=prio)

            def add_group(g, acc, u=8):
                a, b, _, sn = groups[g]
                v = buf.at[pl.ds(base[g], base[g + 1] - base[g])]
                pltpu.make_async_copy(v, v, copy_sems.at[g]).wait()
                full = (b - a) // u if b - a > 2 * u else 0

                def step(t, s):
                    blk = buf[pl.ds(base[g] + t * (u * sn), u * sn)]
                    return s + jnp.sum(blk.reshape(u, sn, SUB, LANE), axis=0)

                if full:
                    acc = lax.fori_loop(0, full, step, acc)
                return _tree_sum(
                    [acc]
                    + [
                        buf[pl.ds(base[g] + t * sn, sn)]
                        for t in range(full * u, b - a)
                    ]
                )

            for c, prio in seq[:head]:
                start_copy(c, prio)

            my = lax.axis_index("i")
            barrier = pltpu.get_barrier_semaphore()
            for d in (2, 1, 3):
                pl.semaphore_signal(
                    barrier, inc=1,
                    device_id=((my + d) % N_DEV,), device_id_type=MESH,
                )

            def issue(m, carry):
                for c, prio in seq[head:head + N_STREAMS]:
                    start_copy(c, prio, m)
                return carry

            lax.fori_loop(0, n_loop, issue, 0)
            for c, prio in seq[head + N_STREAMS * n_loop:]:
                start_copy(c, prio)

            pl.semaphore_wait(barrier, N_DEV - 1)

            def send(k, d, s0, sn):
                rdma = pltpu.make_async_remote_copy(
                    src_ref=comm.at[0, :, lanes(s0, sn)],
                    dst_ref=comm.at[d, :, lanes(s0, sn)],
                    send_sem=send_sems.at[k],
                    recv_sem=recv_sems.at[k],
                    device_id=((my + d) % N_DEV,),
                    device_id_type=MESH,
                )
                rdma.start()
                return rdma

            acc = jnp.zeros((ct, SUB, LANE), jnp.float32)
            for g in range(len(whole)):
                acc = add_group(g, acc)

            diag = []
            for k, (s0, sn) in enumerate(STAGES):
                tot = add_group(len(whole) + k, acc[s0:s0 + sn])
                rows = [jnp.sum(tot[j], axis=0, keepdims=True) for j in range(sn)]
                comm[0, :, lanes(s0, sn)] = jnp.concatenate(rows, axis=1) * inv_total
                diag.append(send(k, 2, s0, sn))
            right = send(len(STAGES), 1, 0, ct)
            left = send(len(STAGES) + 1, 3, 0, ct)

            for rdma in diag + [right, left]:
                rdma.wait_send()
            right.wait_recv()
            left.wait_recv()

            part = {
                s0: comm[0, :, lanes(s0, sn)]
                + (comm[1, :, lanes(s0, sn)] + comm[3, :, lanes(s0, sn)])
                for stage in STAGES
                for s0, sn, _ in column_runs(*stage)
            }
            for rdma, stage in zip(diag, STAGES):
                rdma.wait_recv()
                for s0, sn, c0 in column_runs(*stage):
                    out_ref[:, lanes(c0, sn)] = part[s0] + comm[2, :, lanes(s0, sn)]

        pl.run_scoped(
            scoped,
            pltpu.SemaphoreType.DMA((len(groups),)),
            pltpu.SemaphoreType.DMA((len(STAGES) + 2,)),
            pltpu.SemaphoreType.DMA((len(STAGES) + 2,)),
        )

    x_tiles = (
        x.reshape(nb, SUB, ct, LANE).transpose(0, 2, 1, 3).reshape(nt, SUB, LANE)
    )
    return pl.pallas_call(
        body,
        out_shape=jax.ShapeDtypeStruct((1, n), jnp.float32),
        in_specs=[pl.BlockSpec(memory_space=pl.ANY)],
        out_specs=pl.BlockSpec(memory_space=pltpu.VMEM),
        scratch_shapes=[
            pltpu.VMEM((nt, SUB, LANE), jnp.float32),
            pltpu.VMEM((N_DEV, 1, n), jnp.float32),
        ],
        compiler_params=pltpu.CompilerParams(
            collective_id=0, vmem_limit_bytes=32 * 1024 * 1024
        ),
    )(x_tiles)
```

```python
import jax
import jax.numpy as jnp
from jax import lax
from jax.experimental import pallas as pl
from jax.experimental.pallas import tpu as pltpu

N_DEV = 4
MESH = pl.DeviceIdType.MESH
SUB, LANE = 8, 128

N_STREAMS = 16
OFFSET = 7
PREFILL = 15
N_SPLIT = 6
STAGES = ((0, 4), (4, 2), (6, 1), (7, 1))


def _tree_sum(vals):
    vals = list(vals)
    while len(vals) > 1:
        nxt = [vals[i] + vals[i + 1] for i in range(0, len(vals) - 1, 2)]
        if len(vals) % 2:
            nxt.append(vals[-1])
        vals = nxt
    return vals[0]


def _lanes(first, count):
    return pl.ds(first * LANE, count * LANE)


def pallas_dist_mean_ax0_shard0_i_m4096_n1024_kernel(
x: jax.Array,
):
    m_per, n = x.shape
    ct = n // LANE
    nb = m_per // SUB
    sb = nb // N_STREAMS
    ns = nb - N_SPLIT
    inv_total = 1.0 / (N_DEV * m_per)

    def column_runs(s0, sn):
        carry, c0 = divmod(s0 + OFFSET, ct)
        k = min(sn, ct - c0)
        return [(s0, k, c0, carry)] + (
            [(s0 + k, sn - k, 0, carry + 1)] if k < sn else []
        )

    cuts = [0, nb // 2, nb - 80, nb - 32, ns]
    whole = [(a, b, 0, ct) for a, b in zip(cuts[:-1], cuts[1:])]
    groups = whole + [(ns, nb, s0, sn) for s0, sn in STAGES]
    nw = len(whole)

    fetches = [(p, g) for g, (a, b, _, _) in enumerate(groups) for p in range(a, b)]
    lo = fetches[0:ns:2] + fetches[ns:]
    hi = fetches[1:ns:2]
    seq = [(f, 1) for f in lo[:PREFILL]]
    for i, f in enumerate(lo[PREFILL:]):
        seq += [(h, 0) for h in hi[i:i + 1]] + [(f, 1)]
    assert sorted(f for f, _ in seq) == sorted(fetches)

    def periods(i, end):
        k = 0
        while i + (k + 1) * N_STREAMS <= end and all(
            seq[i + k * N_STREAMS + q] == ((p + k * N_STREAMS, g), prio) and g < nw
            for q, ((p, g), prio) in enumerate(seq[i:i + N_STREAMS])
        ):
            k += 1
        return k

    def body(x_hbm, out_ref, buf, *rest):
        stage_bufs, comm = rest[:-1], rest[-1]

        def scoped(copy_sems, send_sems, recv_sems):
            def dst_of(g, p):
                if g < nw:
                    return buf, p * SUB
                return stage_bufs[g - nw], (p - ns) * SUB

            def start_fetch(f, prio, m=None):
                p, g = f
                _, _, gs0, gsn = groups[g]
                row = (p % N_STREAMS) * sb + p // N_STREAMS
                dref, dst = dst_of(g, p)
                if m is not None:
                    dst = pl.multiple_of(dst + m * (N_STREAMS * SUB), SUB)
                for s0, sn, c0, carry in column_runs(gs0, gsn):
                    src = (row + carry) % nb * SUB
                    if m is not None:
                        src = pl.multiple_of(src + m * SUB, SUB)
                    pltpu.make_async_copy(
                        x_hbm.at[pl.ds(src, SUB), _lanes(c0, sn)],
                        dref.at[pl.ds(dst, SUB), _lanes(s0 - gs0, sn)],
                        copy_sems.at[g],
                    ).start(priority=prio)

            def issue(i, end):
                while i < end:
                    k = periods(i, end)
                    if k < 3:
                        start_fetch(*seq[i])
                        i += 1
                        continue

                    def period(m, carry, i=i):
                        for f, prio in seq[i:i + N_STREAMS]:
                            start_fetch(f, prio, m)
                        return carry

                    lax.fori_loop(0, k, period, 0)
                    i += k * N_STREAMS

            def add_group(g, acc, u=8):
                a, b, _, sn = groups[g]
                ref, off = dst_of(g, a)
                v = ref.at[pl.ds(off, (b - a) * SUB), :]
                pltpu.make_async_copy(v, v, copy_sems.at[g]).wait()
                full = (b - a) // u if b - a > 2 * u else 0

                def step(t, s):
                    r = pl.multiple_of(off + t * (u * SUB), SUB)
                    blk = ref[pl.ds(r, u * SUB), :]
                    return s + jnp.sum(blk.reshape(u, SUB, sn * LANE), axis=0)

                if full:
                    acc = lax.fori_loop(0, full, step, acc)
                return _tree_sum(
                    [acc]
                    + [
                        ref[pl.ds(off + t * SUB, SUB), :]
                        for t in range(full * u, b - a)
                    ]
                )

            head = PREFILL + 8
            issue(0, head)

            my = lax.axis_index("i")
            barrier = pltpu.get_barrier_semaphore()
            for d in (2, 1, 3):
                pl.semaphore_signal(
                    barrier, inc=1,
                    device_id=((my + d) % N_DEV,), device_id_type=MESH,
                )

            mid = cuts[1] + 96
            issue(head, mid)
            acc = add_group(0, jnp.zeros((SUB, n), jnp.float32))
            issue(mid, len(seq))
            for g in range(1, nw):
                acc = add_group(g, acc)

            pl.semaphore_wait(barrier, N_DEV - 1)

            def send(k, d, s0, sn):
                rdma = pltpu.make_async_remote_copy(
                    src_ref=comm.at[0, :, _lanes(s0, sn)],
                    dst_ref=comm.at[d, :, _lanes(s0, sn)],
                    send_sem=send_sems.at[k],
                    recv_sem=recv_sems.at[k],
                    device_id=((my + d) % N_DEV,),
                    device_id_type=MESH,
                )
                rdma.start()
                return rdma

            diag = []
            for k, (s0, sn) in enumerate(STAGES):
                tot = add_group(nw + k, acc[:, s0 * LANE:(s0 + sn) * LANE])
                comm[0, :, _lanes(s0, sn)] = (
                    jnp.sum(tot, axis=0, keepdims=True) * inv_total
                )
                diag.append(send(k, 2, s0, sn))
            right = send(len(STAGES), 1, 0, ct)
            left = send(len(STAGES) + 1, 3, 0, ct)

            for rdma in diag + [right, left]:
                rdma.wait_send()
            right.wait_recv()
            left.wait_recv()

            part = {
                s0: comm[0, :, _lanes(s0, sn)]
                + (comm[1, :, _lanes(s0, sn)] + comm[3, :, _lanes(s0, sn)])
                for stage in STAGES
                for s0, sn, _, _ in column_runs(*stage)
            }
            for rdma, stage in zip(diag, STAGES):
                rdma.wait_recv()
                for s0, sn, c0, _ in column_runs(*stage):
                    out_ref[:, _lanes(c0, sn)] = (
                        part[s0] + comm[2, :, _lanes(s0, sn)]
                    )

        pl.run_scoped(
            scoped,
            pltpu.SemaphoreType.DMA((len(groups),)),
            pltpu.SemaphoreType.DMA((len(STAGES) + 2,)),
            pltpu.SemaphoreType.DMA((len(STAGES) + 2,)),
        )

    return pl.pallas_call(
        body,
        out_shape=jax.ShapeDtypeStruct((1, n), jnp.float32),
        in_specs=[pl.BlockSpec(memory_space=pl.ANY)],
        out_specs=pl.BlockSpec(memory_space=pltpu.VMEM),
        scratch_shapes=[pltpu.VMEM((ns * SUB, n), jnp.float32)]
        + [pltpu.VMEM((N_SPLIT * SUB, sn * LANE), jnp.float32) for _, sn in STAGES]
        + [pltpu.VMEM((N_DEV, 1, n), jnp.float32)],
        compiler_params=pltpu.CompilerParams(
            collective_id=0, vmem_limit_bytes=32 * 1024 * 1024
        ),
    )(x)
```

```python
import jax
import jax.numpy as jnp
from jax import lax
from jax.experimental import pallas as pl
from jax.experimental.pallas import tpu as pltpu

N_DEV = 4
MESH = pl.DeviceIdType.MESH
SUB, LANE = 8, 128
HI, LO = 0, 1

LOG_STREAMS = 4
OFFSET = 7
PREFILL = 15
N_SPLIT = 6
STAGES = ((0, 4), (4, 2), (6, 1), (7, 1))


def _tree_sum(vals):
    vals = list(vals)
    while len(vals) > 1:
        nxt = [vals[i] + vals[i + 1] for i in range(0, len(vals) - 1, 2)]
        if len(vals) % 2:
            nxt.append(vals[-1])
        vals = nxt
    return vals[0]


def _lanes(first, count):
    return pl.ds(first * LANE, count * LANE)


def _rows(tile_row, count=1):
    if isinstance(tile_row, int):
        return pl.ds(tile_row * SUB, count * SUB)
    return pl.ds(pl.multiple_of(tile_row * SUB, SUB), count * SUB)


def pallas_dist_mean_ax0_shard0_i_m4096_n1024_kernel(
x: jax.Array,
):
    m_per, n = x.shape
    ct = n // LANE
    nb = m_per // SUB
    sb = nb >> LOG_STREAMS
    ns = nb - N_SPLIT
    inv_total = 1.0 / (N_DEV * m_per)

    cuts = (0, nb // 2, nb - 80, nb - 32, ns)
    nw = len(cuts) - 1

    def column_runs(s0, sn):
        carry, c0 = divmod(s0 + OFFSET, ct)
        k = min(sn, ct - c0)
        return [(s0, k, c0, carry)] + (
            [(s0 + k, sn - k, 0, carry + 1)] if k < sn else []
        )

    def body(x_hbm, out_ref, buf, *rest):
        stage_bufs, comm = rest[:-1], rest[-1]

        def scoped(copy_sems, send_sems, recv_sems):
            def fetch(p, first, slots, dst_ref, dst_row, sem, prio):
                row = (p & ((1 << LOG_STREAMS) - 1)) * sb + (p >> LOG_STREAMS)
                for s0, sn, c0, carry in column_runs(first, slots):
                    src_row = row + carry
                    if isinstance(src_row, int):
                        src_row %= nb
                    pltpu.make_async_copy(
                        x_hbm.at[_rows(src_row), _lanes(c0, sn)],
                        dst_ref.at[_rows(dst_row), _lanes(s0 - first, sn)],
                        sem,
                    ).start(priority=prio)

            def fetch_whole(p, prio):
                if isinstance(p, int):
                    g = sum(p >= c for c in cuts[1:-1])
                else:
                    g = sum((p >= c).astype(jnp.int32) for c in cuts[1:-1])
                fetch(p, 0, ct, buf, p, copy_sems.at[g], prio)

            def fetch_stage(j):
                k, q = divmod(j, N_SPLIT)
                fetch(ns + q, *STAGES[k], stage_bufs[k], q, copy_sems.at[nw + k], LO)

            def pair(i, carry):
                fetch_whole(2 * i + 1, HI)
                fetch_whole(2 * (i + PREFILL), LO)
                return carry

            def add(ref, first, count, sem, acc, u=8):
                v = ref.at[_rows(first, count), :]
                pltpu.make_async_copy(v, v, sem).wait()
                full = count // u if count > 2 * u else 0

                def step(t, s):
                    blk = ref[_rows(first + t * u, u), :]
                    return s + jnp.sum(blk.reshape(u, *s.shape), axis=0)

                if full:
                    acc = lax.fori_loop(0, full, step, acc)
                return _tree_sum(
                    [acc] + [ref[_rows(first + t), :] for t in range(full * u, count)]
                )

            def add_whole(g, acc):
                return add(buf, cuts[g], cuts[g + 1] - cuts[g], copy_sems.at[g], acc)

            for i in range(PREFILL):
                fetch_whole(2 * i, LO)
            for i in range(4):
                pair(i, 0)

            my = lax.axis_index("i")
            barrier = pltpu.get_barrier_semaphore()
            for d in (2, 1, 3):
                pl.semaphore_signal(
                    barrier, inc=1,
                    device_id=((my + d) % N_DEV,), device_id_type=MESH,
                )

            mid = cuts[1] // 2 + 40
            n_pairs = ns // 2 - PREFILL
            lax.fori_loop(4, mid, pair, 0)
            acc = add_whole(0, jnp.zeros((SUB, n), jnp.float32))
            lax.fori_loop(mid, n_pairs, pair, 0)
            for j in range(len(STAGES) * N_SPLIT):
                if j < PREFILL:
                    fetch_whole(2 * (n_pairs + j) + 1, HI)
                fetch_stage(j)
            for g in range(1, nw):
                acc = add_whole(g, acc)

            pl.semaphore_wait(barrier, N_DEV - 1)

            def send(k, d, s0, sn):
                rdma = pltpu.make_async_remote_copy(
                    src_ref=comm.at[0, :, _lanes(s0, sn)],
                    dst_ref=comm.at[d, :, _lanes(s0, sn)],
                    send_sem=send_sems.at[k],
                    recv_sem=recv_sems.at[k],
                    device_id=((my + d) % N_DEV,),
                    device_id_type=MESH,
                )
                rdma.start()
                return rdma

            diag = []
            for k, (s0, sn) in enumerate(STAGES):
                tot = add(
                    stage_bufs[k], 0, N_SPLIT, copy_sems.at[nw + k],
                    acc[:, s0 * LANE:(s0 + sn) * LANE],
                )
                comm[0, :, _lanes(s0, sn)] = (
                    jnp.sum(tot, axis=0, keepdims=True) * inv_total
                )
                diag.append(send(k, 2, s0, sn))
            right = send(len(STAGES), 1, 0, ct)
            left = send(len(STAGES) + 1, 3, 0, ct)

            for rdma in diag + [right, left]:
                rdma.wait_send()
            right.wait_recv()
            left.wait_recv()

            part = {
                s0: comm[0, :, _lanes(s0, sn)]
                + (comm[1, :, _lanes(s0, sn)] + comm[3, :, _lanes(s0, sn)])
                for stage in STAGES
                for s0, sn, _, _ in column_runs(*stage)
            }
            for rdma, stage in zip(diag, STAGES):
                rdma.wait_recv()
                for s0, sn, c0, _ in column_runs(*stage):
                    out_ref[:, _lanes(c0, sn)] = (
                        part[s0] + comm[2, :, _lanes(s0, sn)]
                    )

        pl.run_scoped(
            scoped,
            pltpu.SemaphoreType.DMA((nw + len(STAGES),)),
            pltpu.SemaphoreType.DMA((len(STAGES) + 2,)),
            pltpu.SemaphoreType.DMA((len(STAGES) + 2,)),
        )

    return pl.pallas_call(
        body,
        out_shape=jax.ShapeDtypeStruct((1, n), jnp.float32),
        in_specs=[pl.BlockSpec(memory_space=pl.ANY)],
        out_specs=pl.BlockSpec(memory_space=pltpu.VMEM),
        scratch_shapes=[pltpu.VMEM((ns * SUB, n), jnp.float32)]
        + [pltpu.VMEM((N_SPLIT * SUB, sn * LANE), jnp.float32) for _, sn in STAGES]
        + [pltpu.VMEM((N_DEV, 1, n), jnp.float32)],
        compiler_params=pltpu.CompilerParams(
            collective_id=0, vmem_limit_bytes=32 * 1024 * 1024
        ),
    )(x)
```

```python
import jax
import jax.numpy as jnp
from jax import lax
from jax.experimental import pallas as pl
from jax.experimental.pallas import tpu as pltpu

N_DEV = 4
MESH = pl.DeviceIdType.MESH
SUB, LANE = 8, 128
HI, LO = 0, 1

LOG_STREAMS = 4
OFFSET = 7
PREFILL = 15
N_SPLIT = 6
STAGES = ((0, 4), (4, 2), (6, 1), (7, 1))


def _tree_sum(vals):
    vals = list(vals)
    while len(vals) > 1:
        nxt = [vals[i] + vals[i + 1] for i in range(0, len(vals) - 1, 2)]
        if len(vals) % 2:
            nxt.append(vals[-1])
        vals = nxt
    return vals[0]


def _lanes(first, count):
    return pl.ds(first * LANE, count * LANE)


def _rows(tile_row, count=1):
    if isinstance(tile_row, int):
        return pl.ds(tile_row * SUB, count * SUB)
    return pl.ds(pl.multiple_of(tile_row * SUB, SUB), count * SUB)


def pallas_dist_mean_ax0_shard0_i_m4096_n1024_kernel(
x: jax.Array,
):
    m_per, n = x.shape
    ct = n // LANE
    nb = m_per // SUB
    sb = nb >> LOG_STREAMS
    ns = nb - N_SPLIT
    inv_total = 1.0 / (N_DEV * m_per)

    cuts = (0, nb // 2, nb - 80, nb - 32, ns)
    nw = len(cuts) - 1
    assert nb & (nb - 1) == 0 and all(c % 2 == 0 for c in cuts)

    def column_runs(s0, sn):
        carry, c0 = divmod(s0 + OFFSET, ct)
        k = min(sn, ct - c0)
        return [(s0, k, c0, carry)] + (
            [(s0 + k, sn - k, 0, carry + 1)] if k < sn else []
        )

    def body(x_hbm, out_ref, buf, *rest):
        stage_bufs, comm = rest[:-1], rest[-1]

        def scoped(copy_sems, send_sems, recv_sems):
            def fetch(p, first, slots, dst_ref, dst_row, sem, prio):
                row = (p & ((1 << LOG_STREAMS) - 1)) * sb + (p >> LOG_STREAMS)
                for s0, sn, c0, carry in column_runs(first, slots):
                    src_row = (row + carry) & (nb - 1)
                    pltpu.make_async_copy(
                        x_hbm.at[_rows(src_row), _lanes(c0, sn)],
                        dst_ref.at[_rows(dst_row), _lanes(s0 - first, sn)],
                        sem,
                    ).start(priority=prio)

            def fetch_whole(p, prio, step=0):
                sem = copy_sems.at[sum(p >= c for c in cuts[1:-1])]
                fetch(p + step, 0, ct, buf, p + step, sem, prio)

            def fetch_stage(j):
                k, q = divmod(j, N_SPLIT)
                fetch(ns + q, *STAGES[k], stage_bufs[k], q, copy_sems.at[nw + k], LO)

            def fetch_pairs(i0, i1):
                edges = {i0, i1}
                for c in cuts[1:-1]:
                    edges |= {e for e in (c // 2, c // 2 - PREFILL) if i0 < e < i1}
                edges = sorted(edges)
                for a, b in zip(edges[:-1], edges[1:]):
                    def pair(i, carry, a=a):
                        fetch_whole(2 * a + 1, HI, 2 * i)
                        fetch_whole(2 * (a + PREFILL), LO, 2 * i)
                        return carry

                    lax.fori_loop(0, b - a, pair, 0)

            def add(ref, first, count, sem, acc, u=8):
                v = ref.at[_rows(first, count), :]
                pltpu.make_async_copy(v, v, sem).wait()
                full = count // u if count > 2 * u else 0

                def step(t, s):
                    blk = ref[_rows(first + t * u, u), :]
                    return s + jnp.sum(blk.reshape(u, *s.shape), axis=0)

                if full:
                    acc = lax.fori_loop(0, full, step, acc)
                return _tree_sum(
                    [acc] + [ref[_rows(first + t), :] for t in range(full * u, count)]
                )

            def add_whole(g, acc):
                return add(buf, cuts[g], cuts[g + 1] - cuts[g], copy_sems.at[g], acc)

            for i in range(PREFILL):
                fetch_whole(2 * i, LO)
            fetch_pairs(0, 4)

            my = lax.axis_index("i")
            barrier = pltpu.get_barrier_semaphore()
            for d in (2, 1, 3):
                pl.semaphore_signal(
                    barrier, inc=1,
                    device_id=((my + d) % N_DEV,), device_id_type=MESH,
                )

            mid = cuts[1] // 2 + 40
            n_pairs = ns // 2 - PREFILL
            fetch_pairs(4, mid)
            acc = add_whole(0, jnp.zeros((SUB, n), jnp.float32))
            fetch_pairs(mid, n_pairs)
            for j in range(len(STAGES) * N_SPLIT):
                if j < PREFILL:
                    fetch_whole(2 * (n_pairs + j) + 1, HI)
                fetch_stage(j)

            pl.semaphore_wait(barrier, N_DEV - 1)

            for g in range(1, nw):
                acc = add_whole(g, acc)

            def send(k, d, s0, sn):
                rdma = pltpu.make_async_remote_copy(
                    src_ref=comm.at[0, :, _lanes(s0, sn)],
                    dst_ref=comm.at[d, :, _lanes(s0, sn)],
                    send_sem=send_sems.at[k],
                    recv_sem=recv_sems.at[k],
                    device_id=((my + d) % N_DEV,),
                    device_id_type=MESH,
                )
                rdma.start()
                return rdma

            diag = []
            for k, (s0, sn) in enumerate(STAGES):
                tot = add(
                    stage_bufs[k], 0, N_SPLIT, copy_sems.at[nw + k],
                    acc[:, s0 * LANE:(s0 + sn) * LANE],
                )
                comm[0, :, _lanes(s0, sn)] = (
                    jnp.sum(tot, axis=0, keepdims=True) * inv_total
                )
                diag.append(send(k, 2, s0, sn))
            right = send(len(STAGES), 1, 0, ct)
            left = send(len(STAGES) + 1, 3, 0, ct)

            for rdma in diag + [right, left]:
                rdma.wait_send()
            right.wait_recv()
            left.wait_recv()

            part = {
                s0: comm[0, :, _lanes(s0, sn)]
                + (comm[1, :, _lanes(s0, sn)] + comm[3, :, _lanes(s0, sn)])
                for stage in STAGES
                for s0, sn, _, _ in column_runs(*stage)
            }
            for rdma, stage in zip(diag, STAGES):
                rdma.wait_recv()
                for s0, sn, c0, _ in column_runs(*stage):
                    out_ref[:, _lanes(c0, sn)] = (
                        part[s0] + comm[2, :, _lanes(s0, sn)]
                    )

        pl.run_scoped(
            scoped,
            pltpu.SemaphoreType.DMA((nw + len(STAGES),)),
            pltpu.SemaphoreType.DMA((len(STAGES) + 2,)),
            pltpu.SemaphoreType.DMA((len(STAGES) + 2,)),
        )

    return pl.pallas_call(
        body,
        out_shape=jax.ShapeDtypeStruct((1, n), jnp.float32),
        in_specs=[pl.BlockSpec(memory_space=pl.ANY)],
        out_specs=pl.BlockSpec(memory_space=pltpu.VMEM),
        scratch_shapes=[pltpu.VMEM((ns * SUB, n), jnp.float32)]
        + [pltpu.VMEM((N_SPLIT * SUB, sn * LANE), jnp.float32) for _, sn in STAGES]
        + [pltpu.VMEM((N_DEV, 1, n), jnp.float32)],
        compiler_params=pltpu.CompilerParams(
            collective_id=0, vmem_limit_bytes=32 * 1024 * 1024
        ),
    )(x)
```
